```python
import numpy as np

kernel_name = "dist_rope_attn_qseq_b2_sq128_d512_hq4_dh64"

def setup_inputs():
    x = np.random.randn(2, 512, 512).astype(np.float32)
    Wq = np.random.randn(512, 256).astype(np.float32) * 0.02
    Wk = np.random.randn(512, 256).astype(np.float32) * 0.02
    Wv = np.random.randn(512, 256).astype(np.float32) * 0.02
    Wo = np.random.randn(256, 512).astype(np.float32) * 0.02
    return {"x": x, "Wq": Wq, "Wk": Wk, "Wv": Wv, "Wo": Wo}

def reference(x, Wq, Wk, Wv, Wo):
    B, Sq, Hq, Dh = 2, 512, 4, 64
    inv = 1.0 / (10000.0 ** (np.arange(0, Dh, 2) / Dh))
    pos = np.arange(Sq)[:, None] * inv[None, :]
    cos = np.repeat(np.cos(pos), 2, axis=-1).astype(np.float32)
    sin = np.repeat(np.sin(pos), 2, axis=-1).astype(np.float32)
    def rot(t):
        t2 = t.reshape(B, Sq, Hq, Dh // 2, 2)
        t_r = np.stack([-t2[..., 1], t2[..., 0]], axis=-1).reshape(B, Sq, Hq, Dh)
        return t * cos[None, :, None, :] + t_r * sin[None, :, None, :]
    Q = rot((x @ Wq).reshape(B, Sq, Hq, Dh))
    K = rot((x @ Wk).reshape(B, Sq, Hq, Dh))
    V = (x @ Wv).reshape(B, Sq, Hq, Dh)
    s = np.einsum('bihd,bjhd->bhij', Q, K).astype(np.float32) * 0.125
    s_max = s.max(axis=-1, keepdims=True)
    w = np.exp(s - s_max)
    w = w / w.sum(axis=-1, keepdims=True)
    ctx = np.einsum('bhij,bjhd->bihd', w, V).reshape(B, Sq, Hq * Dh)
    return ctx @ Wo
```

```python
import math
import jax
import jax.numpy as jnp
from jax import lax
from jax.experimental import pallas as pl
from jax.experimental.pallas import tpu as pltpu

MESH = pl.DeviceIdType.MESH
LOG2E = 1.4426950408889634
BF = jnp.bfloat16
F32 = jnp.float32


def make_kernel(type_order=(0, 1, 2), d_order=(2, 3, 1), ret_order=(3, 1, 2)):
    def kernel(x, Wq, Wk, Wv, Wo):
        def body(x_ref, wq_ref, wk_ref, wv_ref, wo_ref, o_ref,
                 xf, wf, wof, sbuf, rbuf, cs, cr, pbuf,
                 ld_sems, s_sems, r_sems, cs_sems, cr_sems):
            me = lax.axis_index("i")
            b = me // 2
            hp = me % 2
            bsem = pltpu.get_barrier_semaphore()
            for d in (1, 2, 3):
                pl.semaphore_signal(bsem, inc=1, device_id=(me ^ d,), device_id_type=MESH)

            w_refs = (wq_ref, wk_ref, wv_ref)
            def xcopy(rel):
                bb = b ^ 1 if rel == 0 else b
                return pltpu.make_async_copy(x_ref.at[bb], xf.at[rel], ld_sems.at[rel])
            def wcopy(t, rel):
                hh = hp ^ 1 if rel == 0 else hp
                return pltpu.make_async_copy(
                    w_refs[t].at[:, pl.ds(pl.multiple_of(hh * 128, 128), 128)], wf.at[t, rel], ld_sems.at[2 + 2 * t + rel])
            def wocopy(rel):
                hh = hp ^ 1 if rel == 0 else hp
                return pltpu.make_async_copy(
                    wo_ref.at[pl.ds(pl.multiple_of(hh * 128, 128), 128), :], wof.at[rel], ld_sems.at[8 + rel])
            t0 = type_order[0]
            xcopy(0).start(); wcopy(t0, 0).start(); xcopy(1).start(); wcopy(t0, 1).start()
            for t in type_order[1:]:
                wcopy(t, 0).start(); wcopy(t, 1).start()
            wocopy(0).start(); wocopy(1).start()

            lane = lax.broadcasted_iota(jnp.int32, (128, 128), 1)
            row = lax.broadcasted_iota(jnp.int32, (128, 128), 0)
            fidx = ((lane & 63) >> 1).astype(F32)
            inv = jnp.exp(fidx * (-math.log(10000.0) / 32.0))
            ang = (row + me * 128).astype(F32) * inv
            cos = jnp.cos(ang)
            even = (lane & 1) == 0
            sin = jnp.sin(ang)
            sin = jnp.where(even, -sin, sin)

            def rope(t):
                sw = jnp.where(even, pltpu.roll(t, 127, 1), pltpu.roll(t, 1, 1))
                return t * cos + sw * sin

            def tile_src(d):
                xr = 0 if (d >> 1) else 1
                wr = 0 if (d & 1) else 1
                return xr, wr

            x_waited = [False, False]
            w_waited = {}
            xb = [None, None]
            def get_x(rel):
                if not x_waited[rel]:
                    xcopy(rel).wait(); x_waited[rel] = True
                    xb[rel] = xf[rel].astype(BF)
                return xb[rel]
            def get_w(t, rel):
                if (t, rel) not in w_waited:
                    wcopy(t, rel).wait(); w_waited[(t, rel)] = True
                return wf[t, rel].astype(BF)

            def rdma(t, d):
                return pltpu.make_async_remote_copy(
                    sbuf.at[t, d], rbuf.at[t, d], s_sems.at[t * 4 + d], r_sems.at[t * 4 + d],
                    device_id=(me ^ d,), device_id_type=MESH)

            barrier_done = False
            for t in type_order:
                for d in (3, 1, 2, 0):
                    xr, wr = tile_src(d)
                    acc = jnp.dot(get_x(xr), get_w(t, wr), preferred_element_type=F32)
                    if t == 0:
                        acc = rope(acc) * (0.125 * LOG2E)
                    elif t == 1:
                        acc = rope(acc)
                    if d == 0:
                        rbuf[t, 0] = acc.astype(BF)
                    else:
                        sbuf[t, d] = acc.astype(BF)
                if not barrier_done:
                    pl.semaphore_wait(bsem, 3)
                    barrier_done = True
                for d in d_order:
                    rdma(t, d).start()

            for t in (0, 1):
                for d in (1, 2, 3):
                    rdma(t, d).wait_recv()
            kall = rbuf[1].reshape(512, 128)
            lo = lane < 64
            lrec = [[None, None] for _ in range(4)]
            for d in (2, 3, 1, 0):
                q = rbuf[0, d]
                for h in (0, 1):
                    qm = jnp.where(lo if h == 0 else ~lo, q, jnp.zeros_like(q))
                    s = lax.dot_general(qm, kall, (((1,), (1,)), ((), ())), preferred_element_type=F32)
                    m = jnp.max(s, axis=-1, keepdims=True)
                    p = jnp.exp2(s - m)
                    l = jnp.sum(p, axis=-1, keepdims=True)
                    pbuf[d, h] = p.astype(BF)
                    lrec[d][h] = 1.0 / l
            for d in (1, 2, 3):
                rdma(2, d).wait_recv()
            vall = rbuf[2].reshape(512, 128)

            def ret(d):
                return pltpu.make_async_remote_copy(
                    cs.at[d], cr.at[d], cs_sems.at[d], cr_sems.at[d],
                    device_id=(me ^ d,), device_id_type=MESH)
            for d in tuple(ret_order) + (0,):
                o0 = jnp.dot(pbuf[d, 0], vall, preferred_element_type=F32) * lrec[d][0]
                o1 = jnp.dot(pbuf[d, 1], vall, preferred_element_type=F32) * lrec[d][1]
                ctx = jnp.where(lo, o0, o1).astype(BF)
                if d == 0:
                    cr[0] = ctx
                else:
                    cs[d] = ctx
                    ret(d).start()

            wocopy(0).wait(); wocopy(1).wait()
            wo_o = wof[0].astype(BF)
            wo_m = wof[1].astype(BF)
            ret(1).wait_recv()
            o_ref[b] = (jnp.dot(cr[0], wo_m, preferred_element_type=F32)
                        + jnp.dot(cr[1], wo_o, preferred_element_type=F32))
            ret(3).wait_recv()
            ret(2).wait_recv()
            o_ref[b ^ 1] = (jnp.dot(cr[2], wo_m, preferred_element_type=F32)
                            + jnp.dot(cr[3], wo_o, preferred_element_type=F32))
            for d in (1, 2, 3):
                ret(d).wait_send()
            for t in range(3):
                for d in (1, 2, 3):
                    rdma(t, d).wait_send()

        A = pl.BlockSpec(memory_space=pl.ANY)
        return pl.pallas_call(
            body,
            out_shape=jax.ShapeDtypeStruct(x.shape, F32),
            in_specs=[A] * 5,
            out_specs=pl.BlockSpec(memory_space=pltpu.VMEM),
            scratch_shapes=[
                pltpu.VMEM((2, 128, 512), F32),
                pltpu.VMEM((3, 2, 512, 128), F32),
                pltpu.VMEM((2, 128, 512), F32),
                pltpu.VMEM((3, 4, 128, 128), BF),
                pltpu.VMEM((3, 4, 128, 128), BF),
                pltpu.VMEM((4, 128, 128), BF),
                pltpu.VMEM((4, 128, 128), BF),
                pltpu.VMEM((4, 2, 128, 512), BF),
                pltpu.SemaphoreType.DMA((10,)),
                pltpu.SemaphoreType.DMA((12,)),
                pltpu.SemaphoreType.DMA((12,)),
                pltpu.SemaphoreType.DMA((4,)),
                pltpu.SemaphoreType.DMA((4,)),
            ],
            compiler_params=pltpu.CompilerParams(collective_id=0),
        )(x, Wq, Wk, Wv, Wo)
    return kernel


_KERNEL = make_kernel()


def pallas_dist_rope_attn_qseq_b2_sq128_d512_hq4_dh64_kernel(x, Wq, Wk, Wv, Wo):
    return _KERNEL(x, Wq, Wk, Wv, Wo)
```

```python
import math

import jax
import jax.numpy as jnp
from jax import lax
from jax.experimental import pallas as pl
from jax.experimental.pallas import tpu as pltpu

_MESH = pl.DeviceIdType.MESH
_BF = jnp.bfloat16
_F32 = jnp.float32
_NT = (((1,), (1,)), ((), ()))
_V, _K, _Q = 0, 1, 2
_TYPE = {"V": _V, "K": _K, "Q": _Q}
_QSCALE = 0.125 * 1.4426950408889634

_SCHEDULE = {
    0: "TAB TK3 TK1 BAR sK3 TK2 sK1 TV1 sV1 TV3 DG sK2 TQ3 TV2 TQ2 sQ2 TQ1 sV2 TV0 sQ1 TK0 TQ0 sQ3 sV3 "
       "S1 WO PV1 r1 S3 PV3 r3 S0 PV0 S2 PV2 r2 o1 o0 o3 o2",
    3: "TAB BAR TK3 DG sK3 TK1 sK1 TK2 sK2 TV1 TV3 sV3 TQ3 TV2 TQ2 sV2 sQ2 TQ1 sQ3 TV0 TK0 sV1 TQ0 sQ1 "
       "S3 WO PV3 r3 S2 PV2 r2 S1 PV1 r1 S0 PV0 o3 o0 o1 o2",
    1: "TAB BAR TK3 sK3 TK1 DG sK1 TK2 sK2 TV1 sV1 TV3 sV3 TQ3 TV2 sV2 TQ2 sQ2 TQ1 sQ1 TV0 TK0 TQ0 "
       "S1 WO sQ3 PV1 r1 S0 PV0 S2 PV2 r2 S3 PV3 r3 o0 o1 o3 o2",
    2: "TAB BAR TK3 sK3 TK1 sK1 DG TK2 sK2 TV1 sV1 TV3 sV3 TQ3 TV2 sV2 TQ2 sQ2 TQ1 TV0 TK0 sQ3 TQ0 "
       "S2 WO sQ1 PV2 r2 S1 PV1 r1 S3 PV3 r3 S0 PV0 o0 o3 o1 o2",
}


def _parse(schedule):
    shared, scalar = None, {}
    for chip in range(4):
        ops, before = [], {}
        for tok in schedule[chip].split():
            if tok in ("BAR", "DG"):
                before.setdefault(len(ops), []).append((tok, None, None))
            elif tok[0] == "s":
                before.setdefault(len(ops), []).append(("SEND", _TYPE[tok[1]], int(tok[2])))
            elif tok[0] == "r":
                continue
            elif tok in ("TAB", "WO"):
                ops.append((tok, None, None))
            elif tok[0] == "T":
                ops.append(("TILE", _TYPE[tok[1]], int(tok[2])))
            elif tok[:2] == "PV":
                ops.append(("PV", None, int(tok[2])))
            elif tok[0] == "S":
                ops.append(("S", None, int(tok[1])))
            else:
                ops.append(("OUT", None, int(tok[1])))
        if shared is None:
            shared = [(k, t, [d] * 4) for k, t, d in ops]
        assert [o[:2] for o in ops] == [o[:2] for o in shared]
        for j, (_, _, d) in enumerate(ops):
            shared[j][2][chip] = d
        scalar[chip] = before
    return shared, scalar


_SHARED, _SCALAR = _parse(_SCHEDULE)


def _load_groups():
    groups, at, seen = [], {}, set()
    for j, (kind, t, d) in enumerate(_SHARED):
        if kind == "TILE":
            assert len(set(d)) == 1
            need = [("x", d[0] >> 1), ("w", t, d[0] & 1)]
            new = [n for n in need if n not in seen]
            if new:
                seen.update(new)
                at[j] = len(groups)
                groups.append(new)
    groups.append([("wo", 0), ("wo", 1)])
    return groups, at


_GROUPS, _GROUP_AT = _load_groups()


def _body(x_ref, wq_ref, wk_ref, wv_ref, wo_ref, o_ref,
          xf, wf, wof, xbf, wbf, wob, sbuf, rbuf, cbuf, pbuf,
          ld_sems, send_sem, recv_sems, diag_sem):
    me = lax.axis_index("i")
    b = lax.shift_right_logical(me, 1)
    hp = me & 1
    w_refs = (wv_ref, wk_ref, wq_ref)

    def load(spec, sem):
        if spec[0] == "x":
            return pltpu.make_async_copy(x_ref.at[b ^ spec[1]], xf.at[spec[1]], ld_sems.at[sem])
        if spec[0] == "w":
            _, t, s = spec
            cols = pl.ds(pl.multiple_of((hp ^ s) * 128, 128), 128)
            return pltpu.make_async_copy(w_refs[t].at[:, cols], wf.at[t, s], ld_sems.at[sem])
        rows = pl.ds(pl.multiple_of((hp ^ spec[1]) * 128, 128), 128)
        return pltpu.make_async_copy(wo_ref.at[rows, :], wof.at[spec[1]], ld_sems.at[sem])

    barrier = pltpu.get_barrier_semaphore()
    for d in (3, 1):
        pl.semaphore_signal(barrier, inc=1, device_id=(me ^ d,), device_id_type=_MESH)
    loads = [[load(s, i) for s in g] for i, g in enumerate(_GROUPS)]
    for g in loads:
        for c in g:
            c.start()

    def tile_copy(t, d):
        sem = recv_sems.at[t] if t != _Q else recv_sems.at[1 + d]
        return pltpu.make_async_remote_copy(
            sbuf.at[3 * t + d - 1], rbuf.at[t, d], send_sem, sem,
            device_id=(me ^ d,), device_id_type=_MESH)

    def ctx_copy(d):
        return pltpu.make_async_remote_copy(
            sbuf.at[8 + d], cbuf.at[d], send_sem, recv_sems.at[4 + d],
            device_id=(me ^ d,), device_id_type=_MESH)

    def wait_all(t):
        pltpu.make_async_remote_copy(
            rbuf.at[t, pl.ds(1, 3)], rbuf.at[t, pl.ds(1, 3)], send_sem, recv_sems.at[t],
            device_id=(me,), device_id_type=_MESH).wait_recv()

    def peer(d):
        if len(set(d)) == 1:
            return d[0]
        table = sum(v << (2 * chip) for chip, v in enumerate(d))
        return lax.shift_right_logical(jnp.int32(table), 2 * me) & 3

    def if_remote(d, f):
        if isinstance(d, int):
            if d:
                f()
        else:
            pl.when(d != 0)(f)

    def scalar_ops(ops):
        for kind, t, d in ops:
            if kind == "BAR":
                pl.semaphore_wait(barrier, 2)
                pl.semaphore_signal(diag_sem, inc=1, device_id=(me ^ 3,), device_id_type=_MESH)
            elif kind == "DG":
                pl.semaphore_wait(diag_sem, 1)
            else:
                tile_copy(t, d).start()

    def put_ctx(d, ctx):
        def own():
            cbuf[0] = ctx

        def remote():
            sbuf[8 + d] = ctx
            ctx_copy(d).start()
        if isinstance(d, int):
            (remote if d else own)()
        else:
            pl.when(d == 0)(own)
            pl.when(d != 0)(remote)

    lane = lax.broadcasted_iota(jnp.int32, (128, 128), 1)
    even = (lane & 1) == 0
    head0 = lane < 64
    rope_tab = {}

    def rope(t):
        swapped = jnp.where(even, pltpu.roll(t, 127, 1), pltpu.roll(t, 1, 1))
        return t * rope_tab["cos"] + swapped * rope_tab["sin"]

    def scores(d):
        q = rbuf[_Q, d]
        zero = jnp.zeros_like(q)
        qm = jnp.concatenate([jnp.where(head0, q, zero), jnp.where(head0, zero, q)], axis=0)
        s = lax.dot_general(qm, rbuf[_K].reshape(512, 128), _NT, preferred_element_type=_F32)
        p = jnp.exp2(s - jnp.max(s, axis=-1, keepdims=True))
        return p, 1.0 / jnp.sum(p, axis=-1, keepdims=True)

    def pick_heads(o):
        return jnp.where(head0, o[:128], o[128:]).astype(_BF)

    have_k = have_v = False
    done = set()
    n = len(_SHARED)
    for j in range(n + 1):
        if j in done:
            continue
        fused = (j + 1 < n and _SHARED[j][0] == "S" and _SHARED[j + 1][0] == "PV"
                 and _SHARED[j][2] == _SHARED[j + 1][2])
        per_chip = [tuple(_SCALAR[c].get(j, ())) + (tuple(_SCALAR[c].get(j + 1, ())) if fused else ())
                    for c in range(4)]
        if len(set(per_chip)) == 1:
            scalar_ops(per_chip[0])
        else:
            for c in range(4):
                if per_chip[c]:
                    pl.when(me == c)(lambda c=c: scalar_ops(per_chip[c]))
        if j == n:
            break
        kind, t, dl = _SHARED[j]
        if kind == "TAB":
            row = lax.broadcasted_iota(jnp.int32, (128, 128), 0)
            inv_freq = jnp.exp(((lane & 63) >> 1).astype(_F32) * (-math.log(10000.0) / 32.0))
            ang = (row + me * 128).astype(_F32) * inv_freq
            rope_tab["cos"] = jnp.cos(ang)
            sn = jnp.sin(ang)
            rope_tab["sin"] = jnp.where(even, -sn, sn)
            o_ref[...] = jnp.zeros((2, 128, 512), _F32)
        elif kind == "WO":
            for c in loads[-1]:
                c.wait()
            wob[0] = wof[0].astype(_BF)
            wob[1] = wof[1].astype(_BF)
        elif kind == "TILE":
            d = dl[0]
            xs, ws = d >> 1, d & 1
            fresh = ()
            if j in _GROUP_AT:
                for c in loads[_GROUP_AT[j]]:
                    c.wait()
                fresh = _GROUPS[_GROUP_AT[j]]
            if ("x", xs) in fresh:
                xv = xf[xs].astype(_BF)
                xbf[xs] = xv
            else:
                xv = xbf[xs]
            if ("w", t, ws) in fresh:
                wv = wf[t, ws].astype(_BF)
                wbf[t, ws] = wv
            else:
                wv = wbf[t, ws]
            acc = jnp.dot(xv, wv, preferred_element_type=_F32)
            if t == _Q:
                acc = rope(acc) * _QSCALE
            elif t == _K:
                acc = rope(acc)
            if d == 0:
                rbuf[t, 0] = acc.astype(_BF)
            else:
                sbuf[3 * t + d - 1] = acc.astype(_BF)
        elif kind == "S":
            d = peer(dl)
            if not have_k:
                wait_all(_K)
                have_k = True
            if fused and not have_v:
                wait_all(_V)
                have_v = True
            if_remote(d, lambda: tile_copy(_Q, d).wait_recv())
            p, rsum = scores(d)
            if fused:
                done.add(j + 1)
                o = jnp.dot(p.astype(_BF), rbuf[_V].reshape(512, 128), preferred_element_type=_F32)
                put_ctx(d, pick_heads(o * rsum))
            else:
                pbuf[d] = (p * rsum).astype(_BF)
        elif kind == "PV":
            d = peer(dl)
            if not have_v:
                wait_all(_V)
                have_v = True
            o = jnp.dot(pbuf[d], rbuf[_V].reshape(512, 128), preferred_element_type=_F32)
            put_ctx(d, pick_heads(o))
        else:
            d = peer(dl)
            if_remote(d, lambda: ctx_copy(d).wait_recv())
            batch = b ^ lax.shift_right_logical(d, 1)
            o_ref[batch] = o_ref[batch] + jnp.dot(cbuf[d], wob[d & 1], preferred_element_type=_F32)

    pltpu.make_async_remote_copy(
        sbuf, sbuf, send_sem, recv_sems.at[0], device_id=(me,), device_id_type=_MESH).wait_send()


def _kernel(*refs):
    pl.run_scoped(
        lambda *sems: _body(*refs, *sems),
        pltpu.SemaphoreType.DMA((len(_GROUPS),)),
        pltpu.SemaphoreType.DMA,
        pltpu.SemaphoreType.DMA((8,)),
        pltpu.SemaphoreType.REGULAR,
    )


def pallas_dist_rope_attn_qseq_b2_sq128_d512_hq4_dh64_kernel(
    x: jax.Array,
    Wq: jax.Array,
    Wk: jax.Array,
    Wv: jax.Array,
    Wo: jax.Array,
):
    hbm = pl.BlockSpec(memory_space=pl.ANY)
    return pl.pallas_call(
        _kernel,
        out_shape=jax.ShapeDtypeStruct(x.shape, _F32),
        in_specs=[hbm] * 5,
        out_specs=pl.BlockSpec(memory_space=pltpu.VMEM),
        scratch_shapes=[
            pltpu.VMEM((2, 128, 512), _F32),
            pltpu.VMEM((3, 2, 512, 128), _F32),
            pltpu.VMEM((2, 128, 512), _F32),
            pltpu.VMEM((2, 128, 512), _BF),
            pltpu.VMEM((3, 2, 512, 128), _BF),
            pltpu.VMEM((2, 128, 512), _BF),
            pltpu.VMEM((12, 128, 128), _BF),
            pltpu.VMEM((3, 4, 128, 128), _BF),
            pltpu.VMEM((4, 128, 128), _BF),
            pltpu.VMEM((4, 256, 512), _BF),
        ],
        compiler_params=pltpu.CompilerParams(collective_id=0),
    )(x, Wq, Wk, Wv, Wo)
```

```python
import math

import jax
import jax.numpy as jnp
from jax import lax
from jax.experimental import pallas as pl
from jax.experimental.pallas import tpu as pltpu

_MESH = pl.DeviceIdType.MESH
_BF = jnp.bfloat16
_F32 = jnp.float32
_NT = (((1,), (1,)), ((), ()))
_V, _K, _Q = 0, 1, 2
_TYPE = {"V": _V, "K": _K, "Q": _Q}
_QSCALE = 0.125 * 1.4426950408889634

_SCHEDULE = {
    0: "TAB TK3 TK1 BAR sK3 TK2 sK1 TV1 sV1 TV3 DG sK2 TQ3 TV2 TQ2 sQ2 TQ1 sV2 TV0 sQ1 TK0 TQ0 sQ3 sV3 "
       "S1 WO PV1 r1 S3 PV3 r3 S0 PV0 S2 PV2 r2 o1 o0 o3 o2",
    3: "TAB BAR TK3 DG sK3 TK1 sK1 TK2 sK2 TV1 TV3 sV3 TQ3 TV2 TQ2 sV2 sQ2 TQ1 sQ3 TV0 TK0 sV1 TQ0 sQ1 "
       "S3 WO PV3 r3 S2 PV2 r2 S1 PV1 r1 S0 PV0 o3 o0 o1 o2",
    1: "TAB BAR TK3 sK3 TK1 DG sK1 TK2 sK2 TV1 sV1 TV3 sV3 TQ3 TV2 sV2 TQ2 sQ2 TQ1 sQ1 TV0 TK0 TQ0 "
       "S1 WO sQ3 PV1 r1 S0 PV0 S2 PV2 r2 S3 PV3 r3 o0 o1 o3 o2",
    2: "TAB BAR TK3 sK3 TK1 sK1 DG TK2 sK2 TV1 sV1 TV3 sV3 TQ3 TV2 sV2 TQ2 sQ2 TQ1 TV0 TK0 sQ3 TQ0 "
       "S2 WO sQ1 PV2 r2 S1 PV1 r1 S3 PV3 r3 S0 PV0 o0 o3 o1 o2",
}


def _parse(schedule):
    shared, scalar = None, {}
    for chip in range(4):
        ops, before = [], {}
        for tok in schedule[chip].split():
            if tok in ("BAR", "DG"):
                before.setdefault(len(ops), []).append((tok, None, None))
            elif tok[0] == "s":
                before.setdefault(len(ops), []).append(("SEND", _TYPE[tok[1]], int(tok[2])))
            elif tok[0] == "r":
                continue
            elif tok in ("TAB", "WO"):
                ops.append((tok, None, None))
            elif tok[0] == "T":
                ops.append(("TILE", _TYPE[tok[1]], int(tok[2])))
            elif tok[:2] == "PV":
                ops.append(("PV", None, int(tok[2])))
            elif tok[0] == "S":
                ops.append(("S", None, int(tok[1])))
            else:
                ops.append(("OUT", None, int(tok[1])))
        if shared is None:
            shared = [(k, t, [d] * 4) for k, t, d in ops]
        assert [o[:2] for o in ops] == [o[:2] for o in shared]
        for j, (_, _, d) in enumerate(ops):
            shared[j][2][chip] = d
        scalar[chip] = before
    return shared, scalar


_SHARED, _SCALAR = _parse(_SCHEDULE)


def _load_groups():
    groups, at, seen = [], {}, set()
    for j, (kind, t, d) in enumerate(_SHARED):
        if kind == "TILE":
            assert len(set(d)) == 1
            need = [("x", d[0] >> 1), ("w", t, d[0] & 1)]
            new = [n for n in need if n not in seen]
            if new:
                seen.update(new)
                at[j] = len(groups)
                groups.append(new)
    groups.append([("wo", 0), ("wo", 1)])
    return groups, at


_GROUPS, _GROUP_AT = _load_groups()


def _body(x_ref, wq_ref, wk_ref, wv_ref, wo_ref, o_ref,
          xf, wf, wof, xbf, wbf, wob, sbuf, rbuf, cbuf, pbuf,
          far_sems, ld_sems, send_sem, near_sems, diag_sem):
    me = lax.axis_index("i")
    b = lax.shift_right_logical(me, 1)
    hp = me & 1
    w_refs = (wv_ref, wk_ref, wq_ref)

    def load(spec, sem):
        if spec[0] == "x":
            return pltpu.make_async_copy(x_ref.at[b ^ spec[1]], xf.at[spec[1]], ld_sems.at[sem])
        if spec[0] == "w":
            _, t, s = spec
            cols = pl.ds(pl.multiple_of((hp ^ s) * 128, 128), 128)
            return pltpu.make_async_copy(w_refs[t].at[:, cols], wf.at[t, s], ld_sems.at[sem])
        rows = pl.ds(pl.multiple_of((hp ^ spec[1]) * 128, 128), 128)
        return pltpu.make_async_copy(wo_ref.at[rows, :], wof.at[spec[1]], ld_sems.at[sem])

    barrier = pltpu.get_barrier_semaphore()
    for d in (3, 1):
        pl.semaphore_signal(barrier, inc=1, device_id=(me ^ d,), device_id_type=_MESH)
    loads = [[load(s, i) for s in g] for i, g in enumerate(_GROUPS)]
    for g in loads:
        for c in g:
            c.start()

    def recv_sem(base, d):
        if isinstance(d, int) and d == 2:
            return far_sems.at[2 + base]
        return near_sems.at[2 * base + lax.shift_right_logical(d, 1)]

    def tile_copy(t, d):
        sem = far_sems.at[t] if t != _Q else recv_sem(0, d)
        return pltpu.make_async_remote_copy(
            sbuf.at[3 * t + d - 1], rbuf.at[t, d], send_sem, sem,
            device_id=(me ^ d,), device_id_type=_MESH)

    def ctx_copy(d):
        return pltpu.make_async_remote_copy(
            sbuf.at[8 + d], cbuf.at[d], send_sem, recv_sem(1, d),
            device_id=(me ^ d,), device_id_type=_MESH)

    def wait_all(t):
        pltpu.make_async_remote_copy(
            rbuf.at[t, pl.ds(1, 3)], rbuf.at[t, pl.ds(1, 3)], send_sem, far_sems.at[t],
            device_id=(me,), device_id_type=_MESH).wait_recv()

    def peer(d):
        if len(set(d)) == 1:
            return d[0]
        table = sum(v << (2 * chip) for chip, v in enumerate(d))
        return lax.shift_right_logical(jnp.int32(table), 2 * me) & 3

    def if_remote(d, f):
        if isinstance(d, int):
            if d:
                f(d)
        else:
            pl.when(d == 2)(lambda: f(2))
            pl.when((d & 1) == 1)(lambda: f(d))

    def scalar_ops(ops):
        for kind, t, d in ops:
            if kind == "BAR":
                pl.semaphore_wait(barrier, 2)
                pl.semaphore_signal(diag_sem, inc=1, device_id=(me ^ 3,), device_id_type=_MESH)
            elif kind == "DG":
                pl.semaphore_wait(diag_sem, 1)
            else:
                tile_copy(t, d).start()

    def put_ctx(d, ctx):
        def own():
            cbuf[0] = ctx

        def remote(p):
            sbuf[8 + p] = ctx
            ctx_copy(p).start()
        if isinstance(d, int):
            if d == 0:
                own()
        else:
            pl.when(d == 0)(own)
        if_remote(d, remote)

    lane = lax.broadcasted_iota(jnp.int32, (128, 128), 1)
    even = (lane & 1) == 0
    head0 = lane < 64
    rope_tab = {}

    def rope(t):
        swapped = jnp.where(even, pltpu.roll(t, 127, 1), pltpu.roll(t, 1, 1))
        return t * rope_tab["cos"] + swapped * rope_tab["sin"]

    def scores(d):
        q = rbuf[_Q, d]
        zero = jnp.zeros_like(q)
        qm = jnp.concatenate([jnp.where(head0, q, zero), jnp.where(head0, zero, q)], axis=0)
        s = lax.dot_general(qm, rbuf[_K].reshape(512, 128), _NT, preferred_element_type=_F32)
        p = jnp.exp2(s - jnp.max(s, axis=-1, keepdims=True))
        return p, 1.0 / jnp.sum(p, axis=-1, keepdims=True)

    def pick_heads(o):
        return jnp.where(head0, o[:128], o[128:]).astype(_BF)

    have_k = have_v = False
    done = set()
    n = len(_SHARED)
    for j in range(n + 1):
        if j in done:
            continue
        fused = (j + 1 < n and _SHARED[j][0] == "S" and _SHARED[j + 1][0] == "PV"
                 and _SHARED[j][2] == _SHARED[j + 1][2])
        per_chip = [tuple(_SCALAR[c].get(j, ())) + (tuple(_SCALAR[c].get(j + 1, ())) if fused else ())
                    for c in range(4)]
        if len(set(per_chip)) == 1:
            scalar_ops(per_chip[0])
        else:
            for c in range(4):
                if per_chip[c]:
                    pl.when(me == c)(lambda c=c: scalar_ops(per_chip[c]))
        if j == n:
            break
        kind, t, dl = _SHARED[j]
        if kind == "TAB":
            row = lax.broadcasted_iota(jnp.int32, (128, 128), 0)
            inv_freq = jnp.exp(((lane & 63) >> 1).astype(_F32) * (-math.log(10000.0) / 32.0))
            ang = (row + me * 128).astype(_F32) * inv_freq
            rope_tab["cos"] = jnp.cos(ang)
            sn = jnp.sin(ang)
            rope_tab["sin"] = jnp.where(even, -sn, sn)
            o_ref[...] = jnp.zeros((2, 128, 512), _F32)
        elif kind == "WO":
            for c in loads[-1]:
                c.wait()
            wob[0] = wof[0].astype(_BF)
            wob[1] = wof[1].astype(_BF)
        elif kind == "TILE":
            d = dl[0]
            xs, ws = d >> 1, d & 1
            fresh = ()
            if j in _GROUP_AT:
                for c in loads[_GROUP_AT[j]]:
                    c.wait()
                fresh = _GROUPS[_GROUP_AT[j]]
            if ("x", xs) in fresh:
                xv = xf[xs].astype(_BF)
                xbf[xs] = xv
            else:
                xv = xbf[xs]
            if ("w", t, ws) in fresh:
                wv = wf[t, ws].astype(_BF)
                wbf[t, ws] = wv
            else:
                wv = wbf[t, ws]
            acc = jnp.dot(xv, wv, preferred_element_type=_F32)
            if t == _Q:
                acc = rope(acc) * _QSCALE
            elif t == _K:
                acc = rope(acc)
            if d == 0:
                rbuf[t, 0] = acc.astype(_BF)
            else:
                sbuf[3 * t + d - 1] = acc.astype(_BF)
        elif kind == "S":
            d = peer(dl)
            if not have_k:
                wait_all(_K)
                have_k = True
            if fused and not have_v:
                wait_all(_V)
                have_v = True
            if_remote(d, lambda p: tile_copy(_Q, p).wait_recv())
            p, rsum = scores(d)
            if fused:
                done.add(j + 1)
                o = jnp.dot(p.astype(_BF), rbuf[_V].reshape(512, 128), preferred_element_type=_F32)
                put_ctx(d, pick_heads(o * rsum))
            else:
                pbuf[d] = (p * rsum).astype(_BF)
        elif kind == "PV":
            d = peer(dl)
            if not have_v:
                wait_all(_V)
                have_v = True
            o = jnp.dot(pbuf[d], rbuf[_V].reshape(512, 128), preferred_element_type=_F32)
            put_ctx(d, pick_heads(o))
        else:
            d = peer(dl)
            if_remote(d, lambda p: ctx_copy(p).wait_recv())
            batch = b ^ lax.shift_right_logical(d, 1)
            o_ref[batch] = o_ref[batch] + jnp.dot(cbuf[d], wob[d & 1], preferred_element_type=_F32)

    pltpu.make_async_remote_copy(
        sbuf, sbuf, send_sem, far_sems.at[0], device_id=(me,), device_id_type=_MESH).wait_send()


def _kernel(*refs):
    pl.run_scoped(
        lambda *sems: _body(*refs, *sems),
        pltpu.SemaphoreType.DMA((len(_GROUPS),)),
        pltpu.SemaphoreType.DMA,
        pltpu.SemaphoreType.DMA((4,)),
        pltpu.SemaphoreType.REGULAR,
    )


def pallas_dist_rope_attn_qseq_b2_sq128_d512_hq4_dh64_kernel(
    x: jax.Array,
    Wq: jax.Array,
    Wk: jax.Array,
    Wv: jax.Array,
    Wo: jax.Array,
):
    hbm = pl.BlockSpec(memory_space=pl.ANY)
    return pl.pallas_call(
        _kernel,
        out_shape=jax.ShapeDtypeStruct(x.shape, _F32),
        in_specs=[hbm] * 5,
        out_specs=pl.BlockSpec(memory_space=pltpu.VMEM),
        scratch_shapes=[
            pltpu.VMEM((2, 128, 512), _F32),
            pltpu.VMEM((3, 2, 512, 128), _F32),
            pltpu.VMEM((2, 128, 512), _F32),
            pltpu.VMEM((2, 128, 512), _BF),
            pltpu.VMEM((3, 2, 512, 128), _BF),
            pltpu.VMEM((2, 128, 512), _BF),
            pltpu.VMEM((12, 128, 128), _BF),
            pltpu.VMEM((3, 4, 128, 128), _BF),
            pltpu.VMEM((4, 128, 128), _BF),
            pltpu.VMEM((4, 256, 512), _BF),
            pltpu.SemaphoreType.DMA((4,)),
        ],
        compiler_params=pltpu.CompilerParams(collective_id=0),
    )(x, Wq, Wk, Wv, Wo)
```
